```python
import numpy as np

kernel_name = "dist_rope_attn_qseq_b2_sq128_d512_hq4_dh64"

def setup_inputs():
    x = np.random.randn(2, 512, 512).astype(np.float32)
    Wq = np.random.randn(512, 256).astype(np.float32) * 0.02
    Wk = np.random.randn(512, 256).astype(np.float32) * 0.02
    Wv = np.random.randn(512, 256).astype(np.float32) * 0.02
    Wo = np.random.randn(256, 512).astype(np.float32) * 0.02
    return {"x": x, "Wq": Wq, "Wk": Wk, "Wv": Wv, "Wo": Wo}

def reference(x, Wq, Wk, Wv, Wo):
    B, Sq, Hq, Dh = 2, 512, 4, 64
    inv = 1.0 / (10000.0 ** (np.arange(0, Dh, 2) / Dh))
    pos = np.arange(Sq)[:, None] * inv[None, :]
    cos = np.repeat(np.cos(pos), 2, axis=-1).astype(np.float32)
    sin = np.repeat(np.sin(pos), 2, axis=-1).astype(np.float32)
    def rot(t):
        t2 = t.reshape(B, Sq, Hq, Dh // 2, 2)
        t_r = np.stack([-t2[..., 1], t2[..., 0]], axis=-1).reshape(B, Sq, Hq, Dh)
        return t * cos[None, :, None, :] + t_r * sin[None, :, None, :]
    Q = rot((x @ Wq).reshape(B, Sq, Hq, Dh))
    K = rot((x @ Wk).reshape(B, Sq, Hq, Dh))
    V = (x @ Wv).reshape(B, Sq, Hq, Dh)
    s = np.einsum('bihd,bjhd->bhij', Q, K).astype(np.float32) * 0.125
    s_max = s.max(axis=-1, keepdims=True)
    w = np.exp(s - s_max)
    w = w / w.sum(axis=-1, keepdims=True)
    ctx = np.einsum('bhij,bjhd->bihd', w, V).reshape(B, Sq, Hq * Dh)
    return ctx @ Wo
```

```python
import math

import jax
import jax.numpy as jnp
from jax import lax
from jax.experimental import pallas as pl
from jax.experimental.pallas import tpu as pltpu

B, SQ, D, HQ, DH = 2, 128, 512, 4, 64
HD = HQ * DH
NDEV = 4
HALF = 128
BF16 = jnp.bfloat16
F32 = jnp.float32
MESH = pl.DeviceIdType.MESH
PK, PQ, PV = 0, 1, 2


def _scope(name):
    return jax.named_scope(name)


def pallas_dist_rope_attn_qseq_b2_sq128_d512_hq4_dh64_kernel(x, Wq, Wk, Wv, Wo):
    def body(x_hbm, wq_hbm, wk_hbm, wv_hbm, wo_hbm, out_ref,
             x_v, xb_v, wq_v, wk_v, wv_v, wo_v, wo_b, sendbuf, rbuf, p_s, linv_s, ctx_s, ctx_r,
             ld_sems, send_sems, recv_sems, csend_sems, crecv_sems):
        me = lax.axis_index("i")
        beta = me >> 1
        eta = me & 1
        bo = 1 - beta

        loads = [
            pltpu.make_async_copy(x_hbm.at[bo], x_v.at[0], ld_sems.at[0]),
            pltpu.make_async_copy(wk_hbm.at[:, pl.ds(0, HALF)], wk_v.at[:, pl.ds(0, HALF)], ld_sems.at[1]),
            pltpu.make_async_copy(wk_hbm.at[:, pl.ds(HALF, HALF)], wk_v.at[:, pl.ds(HALF, HALF)], ld_sems.at[2]),
            pltpu.make_async_copy(x_hbm.at[beta], x_v.at[1], ld_sems.at[3]),
            pltpu.make_async_copy(wq_hbm, wq_v, ld_sems.at[4]),
            pltpu.make_async_copy(wv_hbm, wv_v, ld_sems.at[5]),
            pltpu.make_async_copy(wo_hbm, wo_v, ld_sems.at[6]),
        ]
        for c in loads:
            c.start()

        bar = pltpu.get_barrier_semaphore()
        for d in (1, 2, 3):
            pl.semaphore_signal(bar, inc=1, device_id=((me + d) % NDEV,), device_id_type=MESH)

        with _scope("tables"):
            lane = lax.broadcasted_iota(jnp.int32, (SQ, HALF), 1)
            fi = (lane & (DH - 1)) >> 1
            inv = jnp.exp(fi.astype(F32) * (-math.log(10000.0) / (DH // 2)))
            pos = (me * SQ + lax.broadcasted_iota(jnp.int32, (SQ, HALF), 0)).astype(F32)
            ang = pos * inv
            cos = jnp.cos(ang)
            even = (lane & 1) == 0
            sin = jnp.sin(ang)
            sin = jnp.where(even, -sin, sin)
            lo = lane < DH

        def rope(t):
            sw = jnp.where(even, pltpu.roll(t, HALF - 1, 1), pltpu.roll(t, 1, 1))
            return t * cos + sw * sin

        def remote(piece, e, slot, dest):
            return pltpu.make_async_remote_copy(
                src_ref=sendbuf.at[piece, slot, e],
                dst_ref=rbuf.at[piece, me],
                send_sem=send_sems.at[piece * 4 + slot * 2 + e],
                recv_sem=recv_sems.at[piece * 4 + me],
                device_id=(dest,), device_id_type=MESH)

        def recv_wait(piece, src):
            pltpu.make_async_remote_copy(
                src_ref=rbuf.at[piece, src], dst_ref=rbuf.at[piece, src],
                send_sem=send_sems.at[0], recv_sem=recv_sems.at[piece * 4 + src],
                device_id=(src,), device_id_type=MESH).wait_recv()

        def emit(piece, slot, e, val):
            b = bo if slot == 0 else beta
            dest = 2 * b + e
            vb = val.astype(BF16)
            if slot == 0:
                sendbuf[piece, slot, e] = vb
                remote(piece, e, slot, dest).start()
            else:
                @pl.when(eta == e)
                def _():
                    rbuf[piece, me] = vb

                @pl.when(eta != e)
                def _():
                    sendbuf[piece, slot, e] = vb
                    remote(piece, e, slot, dest).start()

        def proj_half(slot, w_v, e):
            return jnp.dot(xb_v[slot * SQ:(slot + 1) * SQ, :],
                           w_v[:, e * HALF:(e + 1) * HALF].astype(BF16),
                           preferred_element_type=F32)

        def proj_all(w_v):
            return jnp.dot(xb_v[...], w_v[...].astype(BF16), preferred_element_type=F32)

        def part(t, slot, e):
            return t[slot * SQ:(slot + 1) * SQ, e * HALF:(e + 1) * HALF]

        with _scope("ld_x0_wk0"):
            loads[0].wait()
            loads[1].wait()
        with _scope("k00"):
            xb_v[0:SQ, :] = x_v[0].astype(BF16)
            k = rope(proj_half(0, wk_v, 0))
        with _scope("barrier"):
            pl.semaphore_wait(bar, NDEV - 1)
        with _scope("k00b"):
            emit(PK, 0, 0, k)
        with _scope("ld_wk1"):
            loads[2].wait()
        with _scope("k01"):
            emit(PK, 0, 1, rope(proj_half(0, wk_v, 1)))
        with _scope("ld_x1"):
            loads[3].wait()
        with _scope("k1"):
            xb_v[SQ:2 * SQ, :] = x_v[1].astype(BF16)
            k1 = jnp.dot(xb_v[SQ:2 * SQ, :], wk_v[...].astype(BF16), preferred_element_type=F32)
            for e in range(2):
                emit(PK, 1, e, rope(k1[:, e * HALF:(e + 1) * HALF]))
        with _scope("ld_wq"):
            loads[4].wait()
        with _scope("q"):
            qa = proj_all(wq_v)
            for slot in range(2):
                for e in range(2):
                    emit(PQ, slot, e, rope(part(qa, slot, e)) * 0.125)
        with _scope("ld_wv"):
            loads[5].wait()
        with _scope("v"):
            va = proj_all(wv_v)
            for slot in range(2):
                for e in range(2):
                    emit(PV, slot, e, part(va, slot, e))

        with _scope("wait_k"):
            for d in (1, 2, 3):
                recv_wait(PK, (me + d) % NDEV)

        def scores(d):
            src = (me + d) % NDEV
            q = rbuf[PQ, src]
            zero = jnp.zeros_like(q)
            q2 = jnp.concatenate([jnp.where(lo, q, zero), jnp.where(lo, zero, q)], axis=0)
            kk = rbuf[PK].reshape(NDEV * SQ, HALF)
            s = lax.dot_general(q2, kk, (((1,), (1,)), ((), ())), preferred_element_type=F32)
            m = jnp.max(s, axis=1, keepdims=True)
            p = jnp.exp(s - m)
            l = jnp.sum(p, axis=1, keepdims=True)
            p_s[d] = p.astype(BF16)
            linv_s[d] = jnp.broadcast_to(1.0 / l, (2 * SQ, HALF))

        with _scope("sc0"):
            scores(0)
        for d in (1, 3, 2):
            with _scope(f"wait_q{d}"):
                recv_wait(PQ, (me + d) % NDEV)
            with _scope(f"sc{d}"):
                scores(d)

        with _scope("ld_wo"):
            loads[6].wait()
            wo_b[...] = wo_v[...].astype(BF16)

        with _scope("wait_v"):
            for d in (1, 2, 3):
                recv_wait(PV, (me + d) % NDEV)

        def pv(d):
            vv = rbuf[PV].reshape(NDEV * SQ, HALF)
            o = jnp.dot(p_s[d], vv, preferred_element_type=F32) * linv_s[d]
            return jnp.where(lo, o[:SQ], o[SQ:]).astype(BF16)

        def ctx_copy(dst):
            return pltpu.make_async_remote_copy(
                src_ref=ctx_s.at[dst], dst_ref=ctx_r.at[me],
                send_sem=csend_sems.at[dst], recv_sem=crecv_sems.at[me],
                device_id=(dst,), device_id_type=MESH)

        for d in (2, 1, 3):
            with _scope(f"pv{d}"):
                dst = (me + d) % NDEV
                ctx_s[dst] = pv(d)
                ctx_copy(dst).start()
        with _scope("pv0"):
            ctx_r[me] = pv(0)

        def wo_part(w):
            rows = pl.ds(pl.multiple_of((w & 1) * HALF, HALF), HALF)
            return jnp.dot(ctx_r[w], wo_b[rows, :], preferred_element_type=F32)

        def wait_ctx(w):
            pltpu.make_async_remote_copy(
                src_ref=ctx_s.at[w], dst_ref=ctx_r.at[w],
                send_sem=csend_sems.at[w], recv_sem=crecv_sems.at[w],
                device_id=(w,), device_id_type=MESH).wait_recv()

        with _scope("op_own"):
            out_ref[beta] = wo_part(me)
        sib = me ^ 1
        with _scope("wait_sib"):
            wait_ctx(sib)
        with _scope("op_sib"):
            out_ref[beta] = out_ref[beta] + wo_part(sib)
        with _scope("wait_o1"):
            wait_ctx(2 * bo)
        with _scope("op_o1"):
            out_ref[bo] = wo_part(2 * bo)
        with _scope("wait_o2"):
            wait_ctx(2 * bo + 1)
        with _scope("op_o2"):
            out_ref[bo] = out_ref[bo] + wo_part(2 * bo + 1)
        with _scope("drain"):
            for piece in range(3):
                for slot in range(2):
                    for e in range(2):
                        if slot == 0:
                            remote(piece, e, slot, 0).wait_send()
                        else:
                            @pl.when(eta != e)
                            def _():
                                remote(piece, e, slot, 0).wait_send()
            for d in (1, 2, 3):
                ctx_copy((me + d) % NDEV).wait_send()

    return pl.pallas_call(
        body,
        out_shape=jax.ShapeDtypeStruct((B, SQ, D), F32),
        in_specs=[pl.BlockSpec(memory_space=pl.ANY)] * 5,
        out_specs=pl.BlockSpec(memory_space=pltpu.VMEM),
        scratch_shapes=[
            pltpu.VMEM((B, SQ, D), F32),
            pltpu.VMEM((B * SQ, D), BF16),
            pltpu.VMEM((D, HD), F32),
            pltpu.VMEM((D, HD), F32),
            pltpu.VMEM((D, HD), F32),
            pltpu.VMEM((HD, D), F32),
            pltpu.VMEM((HD, D), BF16),
            pltpu.VMEM((3, 2, 2, SQ, HALF), BF16),
            pltpu.VMEM((3, NDEV, SQ, HALF), BF16),
            pltpu.VMEM((NDEV, 2 * SQ, NDEV * SQ), BF16),
            pltpu.VMEM((NDEV, 2 * SQ, HALF), F32),
            pltpu.VMEM((NDEV, SQ, HALF), BF16),
            pltpu.VMEM((NDEV, SQ, HALF), BF16),
            pltpu.SemaphoreType.DMA((7,)),
            pltpu.SemaphoreType.DMA((12,)),
            pltpu.SemaphoreType.DMA((12,)),
            pltpu.SemaphoreType.DMA((NDEV,)),
            pltpu.SemaphoreType.DMA((NDEV,)),
        ],
        compiler_params=pltpu.CompilerParams(collective_id=0),
    )(x, Wq, Wk, Wv, Wo)
```

```python
import math

import jax
import jax.numpy as jnp
from jax import lax
from jax.experimental import pallas as pl
from jax.experimental.pallas import tpu as pltpu

B, SQ, D, HQ, DH = 2, 128, 512, 4, 64
HD = HQ * DH
NDEV = 4
HALF = 128
BF16 = jnp.bfloat16
F32 = jnp.float32
MESH = pl.DeviceIdType.MESH
PK, PQ, PV = 0, 1, 2


def pallas_dist_rope_attn_qseq_b2_sq128_d512_hq4_dh64_kernel(x, Wq, Wk, Wv, Wo):
    def body(x_hbm, wq_hbm, wk_hbm, wv_hbm, wo_hbm, out_ref,
             x_v, xb_v, wq_v, wk_v, wv_v, wo_v, wo_b, sendbuf, rbuf, p_s, linv_s,
             ctx_s, ctx_r, ld_sems, send_sems, recv_sems, csend_sems, crecv_sems):
        me = lax.axis_index("i")
        beta = me >> 1
        eta = me & 1
        bo = 1 - beta

        loads = [
            pltpu.make_async_copy(x_hbm.at[bo], x_v.at[0], ld_sems.at[0]),
            pltpu.make_async_copy(wk_hbm.at[:, pl.ds(0, HALF)], wk_v.at[:, pl.ds(0, HALF)], ld_sems.at[1]),
            pltpu.make_async_copy(wk_hbm.at[:, pl.ds(HALF, HALF)], wk_v.at[:, pl.ds(HALF, HALF)], ld_sems.at[2]),
            pltpu.make_async_copy(x_hbm.at[beta], x_v.at[1], ld_sems.at[3]),
            pltpu.make_async_copy(wq_hbm, wq_v, ld_sems.at[4]),
            pltpu.make_async_copy(wv_hbm, wv_v, ld_sems.at[5]),
            pltpu.make_async_copy(wo_hbm, wo_v, ld_sems.at[6]),
        ]
        for c in loads:
            c.start()

        bar = pltpu.get_barrier_semaphore()
        for d in (1, 2, 3):
            pl.semaphore_signal(bar, inc=1, device_id=((me + d) % NDEV,), device_id_type=MESH)

        lane = lax.broadcasted_iota(jnp.int32, (SQ, HALF), 1)
        fi = (lane & (DH - 1)) >> 1
        inv = jnp.exp(fi.astype(F32) * (-math.log(10000.0) / (DH // 2)))
        pos = (me * SQ + lax.broadcasted_iota(jnp.int32, (SQ, HALF), 0)).astype(F32)
        ang = pos * inv
        cos = jnp.cos(ang)
        even = (lane & 1) == 0
        sin = jnp.sin(ang)
        sin = jnp.where(even, -sin, sin)
        lo = lane < DH

        def rope(t):
            sw = jnp.where(even, pltpu.roll(t, HALF - 1, 1), pltpu.roll(t, 1, 1))
            return t * cos + sw * sin

        def remote(piece, e, slot, dest):
            return pltpu.make_async_remote_copy(
                src_ref=sendbuf.at[piece, slot, e],
                dst_ref=rbuf.at[piece, me],
                send_sem=send_sems.at[piece * 4 + slot * 2 + e],
                recv_sem=recv_sems.at[piece * 4 + me],
                device_id=(dest,), device_id_type=MESH)

        def recv_wait(piece, src):
            pltpu.make_async_remote_copy(
                src_ref=rbuf.at[piece, src], dst_ref=rbuf.at[piece, src],
                send_sem=send_sems.at[0], recv_sem=recv_sems.at[piece * 4 + src],
                device_id=(src,), device_id_type=MESH).wait_recv()

        def emit(piece, slot, e, val):
            b = bo if slot == 0 else beta
            dest = 2 * b + e
            vb = val.astype(BF16)
            if slot == 0:
                sendbuf[piece, slot, e] = vb
                remote(piece, e, slot, dest).start()
            else:
                @pl.when(eta == e)
                def _():
                    rbuf[piece, me] = vb

                @pl.when(eta != e)
                def _():
                    sendbuf[piece, slot, e] = vb
                    remote(piece, e, slot, dest).start()

        def proj_half(slot, w_v, e):
            return jnp.dot(xb_v[slot * SQ:(slot + 1) * SQ, :],
                           w_v[:, e * HALF:(e + 1) * HALF].astype(BF16),
                           preferred_element_type=F32)

        def proj_all(w_v):
            return jnp.dot(xb_v[...], w_v[...].astype(BF16), preferred_element_type=F32)

        def part(t, slot, e):
            return t[slot * SQ:(slot + 1) * SQ, e * HALF:(e + 1) * HALF]

        loads[0].wait()
        loads[1].wait()
        xb_v[0:SQ, :] = x_v[0].astype(BF16)
        k = rope(proj_half(0, wk_v, 0))
        pl.semaphore_wait(bar, NDEV - 1)
        emit(PK, 0, 0, k)
        loads[2].wait()
        emit(PK, 0, 1, rope(proj_half(0, wk_v, 1)))
        loads[3].wait()
        xb_v[SQ:2 * SQ, :] = x_v[1].astype(BF16)
        k1 = jnp.dot(xb_v[SQ:2 * SQ, :], wk_v[...].astype(BF16), preferred_element_type=F32)
        for e in range(2):
            emit(PK, 1, e, rope(k1[:, e * HALF:(e + 1) * HALF]))
        loads[4].wait()
        qa = proj_all(wq_v)
        for slot in range(2):
            for e in range(2):
                emit(PQ, slot, e, rope(part(qa, slot, e)) * 0.125)
        loads[5].wait()
        va = proj_all(wv_v)
        for slot in range(2):
            for e in range(2):
                emit(PV, slot, e, part(va, slot, e))

        for d in (1, 2, 3):
            recv_wait(PK, (me + d) % NDEV)

        def scores(d):
            src = (me + d) % NDEV
            q = rbuf[PQ, src]
            zero = jnp.zeros_like(q)
            q2 = jnp.concatenate([jnp.where(lo, q, zero), jnp.where(lo, zero, q)], axis=0)
            kk = rbuf[PK].reshape(NDEV * SQ, HALF)
            s = lax.dot_general(q2, kk, (((1,), (1,)), ((), ())), preferred_element_type=F32)
            m = jnp.max(s, axis=1, keepdims=True)
            p = jnp.exp(s - m)
            l = jnp.sum(p, axis=1, keepdims=True)
            p_s[d] = p.astype(BF16)
            linv_s[d] = jnp.broadcast_to(1.0 / l, (2 * SQ, HALF))

        for d in (1, 3, 2):
            recv_wait(PQ, (me + d) % NDEV)
            scores(d)

        loads[6].wait()
        wo_b[...] = wo_v[...].astype(BF16)

        for d in (1, 2, 3):
            recv_wait(PV, (me + d) % NDEV)

        def pv(d):
            vv = rbuf[PV].reshape(NDEV * SQ, HALF)
            o = jnp.dot(p_s[d], vv, preferred_element_type=F32) * linv_s[d]
            return jnp.where(lo, o[:SQ], o[SQ:]).astype(BF16)

        def ctx_copy(dst):
            return pltpu.make_async_remote_copy(
                src_ref=ctx_s.at[dst], dst_ref=ctx_r.at[me],
                send_sem=csend_sems.at[dst], recv_sem=crecv_sems.at[me],
                device_id=(dst,), device_id_type=MESH)

        for d in (2, 1, 3):
            dst = (me + d) % NDEV
            ctx_s[dst] = pv(d)
            ctx_copy(dst).start()
        scores(0)
        ctx_r[me] = pv(0)

        def wo_part(w):
            rows = pl.ds(pl.multiple_of((w & 1) * HALF, HALF), HALF)
            return jnp.dot(ctx_r[w], wo_b[rows, :], preferred_element_type=F32)

        def wait_ctx(w):
            pltpu.make_async_remote_copy(
                src_ref=ctx_s.at[w], dst_ref=ctx_r.at[w],
                send_sem=csend_sems.at[w], recv_sem=crecv_sems.at[w],
                device_id=(w,), device_id_type=MESH).wait_recv()

        out_ref[beta] = wo_part(me)
        sib = me ^ 1
        wait_ctx(sib)
        out_ref[beta] = out_ref[beta] + wo_part(sib)
        wait_ctx(2 * bo)
        out_ref[bo] = wo_part(2 * bo)
        wait_ctx(2 * bo + 1)
        out_ref[bo] = out_ref[bo] + wo_part(2 * bo + 1)

        for piece in range(3):
            for slot in range(2):
                for e in range(2):
                    if slot == 0:
                        remote(piece, e, slot, 0).wait_send()
                    else:
                        @pl.when(eta != e)
                        def _():
                            remote(piece, e, slot, 0).wait_send()
        for d in (1, 2, 3):
            ctx_copy((me + d) % NDEV).wait_send()

    return pl.pallas_call(
        body,
        out_shape=jax.ShapeDtypeStruct((B, SQ, D), F32),
        in_specs=[pl.BlockSpec(memory_space=pl.ANY)] * 5,
        out_specs=pl.BlockSpec(memory_space=pltpu.VMEM),
        scratch_shapes=[
            pltpu.VMEM((B, SQ, D), F32),
            pltpu.VMEM((B * SQ, D), BF16),
            pltpu.VMEM((D, HD), F32),
            pltpu.VMEM((D, HD), F32),
            pltpu.VMEM((D, HD), F32),
            pltpu.VMEM((HD, D), F32),
            pltpu.VMEM((HD, D), BF16),
            pltpu.VMEM((3, 2, 2, SQ, HALF), BF16),
            pltpu.VMEM((3, NDEV, SQ, HALF), BF16),
            pltpu.VMEM((NDEV, 2 * SQ, NDEV * SQ), BF16),
            pltpu.VMEM((NDEV, 2 * SQ, HALF), F32),
            pltpu.VMEM((NDEV, SQ, HALF), BF16),
            pltpu.VMEM((NDEV, SQ, HALF), BF16),
            pltpu.SemaphoreType.DMA((7,)),
            pltpu.SemaphoreType.DMA((12,)),
            pltpu.SemaphoreType.DMA((12,)),
            pltpu.SemaphoreType.DMA((NDEV,)),
            pltpu.SemaphoreType.DMA((NDEV,)),
        ],
        compiler_params=pltpu.CompilerParams(collective_id=0),
    )(x, Wq, Wk, Wv, Wo)
```
